```python
import numpy as np

kernel_name = "dist_mean_ax0_shard0_i_m2048_n1024"

def setup_inputs():
    return {"x": np.random.randn(8192, 1024).astype(np.float32)}

def reference(x: np.ndarray) -> np.ndarray:
    return np.mean(x, axis=0, keepdims=True)
```

```python
import jax
import jax.numpy as jnp
from jax import lax
from jax.experimental import pallas as pl
from jax.experimental.pallas import tpu as pltpu

N_DEV = 4
N_CHUNKS = 8


def pallas_dist_mean_ax0_shard0_i_m2048_n1024_kernel(
x: jax.Array,
):
    m, n = x.shape
    rows = m // N_CHUNKS
    scale = 1.0 / (m * N_DEV)

    def kernel_body(x_hbm, out_ref, buf, parts, load_sems, send_sems, recv_sems):
        me = lax.axis_index("i")

        loads = [
            pltpu.make_async_copy(
                x_hbm.at[pl.ds(c * rows, rows)], buf.at[c], load_sems.at[c]
            )
            for c in range(N_CHUNKS)
        ]
        for cp in loads:
            cp.start()

        barrier = pltpu.get_barrier_semaphore()
        for d in range(1, N_DEV):
            pl.semaphore_signal(
                barrier,
                inc=1,
                device_id=((me + d) % N_DEV,),
                device_id_type=pl.DeviceIdType.MESH,
            )

        acc = jnp.zeros((8, n), jnp.float32)
        for c in range(N_CHUNKS):
            loads[c].wait()
            acc = acc + jnp.sum(buf[c].reshape(rows // 8, 8, n), axis=0)
        parts[0] = jnp.sum(acc, axis=0, keepdims=True)

        pl.semaphore_wait(barrier, N_DEV - 1)

        sends = [
            pltpu.make_async_remote_copy(
                src_ref=parts.at[0],
                dst_ref=parts.at[d],
                send_sem=send_sems.at[d - 1],
                recv_sem=recv_sems.at[d - 1],
                device_id=((me + d) % N_DEV,),
                device_id_type=pl.DeviceIdType.MESH,
            )
            for d in (2, 1, 3)
        ]
        for cp in sends:
            cp.start()
        for cp in sends:
            cp.wait_recv()
        out_ref[...] = ((parts[0] + parts[1]) + (parts[2] + parts[3])) * scale
        for cp in sends:
            cp.wait_send()

    return pl.pallas_call(
        kernel_body,
        out_shape=jax.ShapeDtypeStruct((1, n), x.dtype),
        in_specs=[pl.BlockSpec(memory_space=pl.ANY)],
        out_specs=pl.BlockSpec(memory_space=pltpu.VMEM),
        scratch_shapes=[
            pltpu.VMEM((N_CHUNKS, rows, n), jnp.float32),
            pltpu.VMEM((N_DEV, 1, n), jnp.float32),
            pltpu.SemaphoreType.DMA((N_CHUNKS,)),
            pltpu.SemaphoreType.DMA((N_DEV - 1,)),
            pltpu.SemaphoreType.DMA((N_DEV - 1,)),
        ],
        compiler_params=pltpu.CompilerParams(collective_id=0),
    )(x)
```

```python
import jax
import jax.numpy as jnp
from jax import lax
from jax.experimental import pallas as pl
from jax.experimental.pallas import tpu as pltpu

AXIS = "i"
N_DEV = 4
NEIGHBOURS = (1, 3)
DIAGONAL = 2

SUBLANES = 8
SHARED_ROWS = 96
TAIL_ROWS = 48


def _plan(m, n):
    first, last = m * 3 // 4, 32
    middle = m - first - last - TAIL_ROWS - len(NEIGHBOURS) * SHARED_ROWS
    chunks = (first, middle, last)
    groups = (n // 2, n // 4, n // 8, n // 8)
    assert all(r > 0 and r % SUBLANES == 0 for r in chunks), chunks
    assert sum(groups) == n and all(w % 128 == 0 for w in groups), groups
    return chunks, groups


def _starts(sizes):
    return [sum(sizes[:i]) for i in range(len(sizes))]


def _fold_rows(v):
    r, c = v.shape
    return jnp.sum(v.reshape(r // SUBLANES, SUBLANES, c), axis=0)


def _fold_rows_tree(v):
    xs = [v[i : i + SUBLANES] for i in range(0, v.shape[0], SUBLANES)]
    while len(xs) > 1:
        odd = xs[len(xs) // 2 * 2 :]
        xs = [a + b for a, b in zip(xs[0::2], xs[1::2])] + odd
    return xs[0]


def pallas_dist_mean_ax0_shard0_i_m2048_n1024_kernel(
x: jax.Array,
):
    m, n = x.shape
    chunks, groups = _plan(m, n)
    chunk_starts, group_starts = _starts(chunks), _starts(groups)
    tail_start = sum(chunks)
    shared_start = tail_start + TAIL_ROWS
    distances = (*NEIGHBOURS, DIAGONAL)
    scale = 1.0 / (N_DEV * m)

    def kernel_body(
        x_hbm,
        out_ref,
        chunk_bufs,
        tail_bufs,
        shared_buf,
        parts,
        load_sems,
        shared_send_sems,
        shared_recv_sems,
        part_send_sems,
        part_recv_sems,
    ):
        chunk_loads = [
            pltpu.make_async_copy(
                x_hbm.at[pl.ds(start, rows)], chunk_bufs[c], load_sems.at[c]
            )
            for c, (start, rows) in enumerate(zip(chunk_starts, chunks))
        ]
        tail_loads = [
            pltpu.make_async_copy(
                x_hbm.at[pl.ds(tail_start, TAIL_ROWS), pl.ds(start, width)],
                tail_bufs[g],
                load_sems.at[len(chunks) + g],
            )
            for g, (start, width) in enumerate(zip(group_starts, groups))
        ]
        for load in chunk_loads + tail_loads:
            load.start()

        me = lax.axis_index(AXIS)
        peer = {d: ((me + d) & (N_DEV - 1),) for d in distances}

        barrier = pltpu.get_barrier_semaphore()
        for d in distances:
            pl.semaphore_signal(
                barrier,
                inc=1,
                device_id=peer[d],
                device_id_type=pl.DeviceIdType.MESH,
            )
        pl.semaphore_wait(barrier, len(distances))

        shared = [
            pltpu.make_async_remote_copy(
                src_ref=x_hbm.at[pl.ds(shared_start + j * SHARED_ROWS, SHARED_ROWS)],
                dst_ref=shared_buf.at[j],
                send_sem=shared_send_sems.at[j],
                recv_sem=shared_recv_sems.at[j],
                device_id=peer[d],
                device_id_type=pl.DeviceIdType.MESH,
            )
            for j, d in enumerate(NEIGHBOURS)
        ]
        for copy in shared:
            copy.start()

        chunk_loads[0].wait()
        acc = _fold_rows(chunk_bufs[0][...])
        for c in range(1, len(chunks) - 1):
            chunk_loads[c].wait()
            acc += _fold_rows(chunk_bufs[c][...])
        for j, copy in enumerate(shared):
            copy.wait_recv()
            acc += _fold_rows(shared_buf[j])
        for copy in shared:
            copy.wait_send()
        chunk_loads[-1].wait()
        acc += _fold_rows(chunk_bufs[-1][...])

        sends = {
            (g, d): pltpu.make_async_remote_copy(
                src_ref=parts[g].at[0],
                dst_ref=parts[g].at[d],
                send_sem=part_send_sems.at[g * len(distances) + d - 1],
                recv_sem=part_recv_sems.at[g * len(distances) + d - 1],
                device_id=peer[d],
                device_id_type=pl.DeviceIdType.MESH,
            )
            for g in range(len(groups))
            for d in distances
        }
        for g, (start, width) in enumerate(zip(group_starts, groups)):
            tail_loads[g].wait()
            total = acc[:, start : start + width] + _fold_rows_tree(tail_bufs[g][...])
            parts[g][0] = jnp.sum(total, axis=0, keepdims=True)
            sends[g, DIAGONAL].start()
        for g in range(len(groups)):
            for d in NEIGHBOURS:
                sends[g, d].start()
        for copy in sends.values():
            copy.wait_send()

        from_neighbours = []
        for g in range(len(groups)):
            for d in NEIGHBOURS:
                sends[g, d].wait_recv()
            from_neighbours.append(parts[g][NEIGHBOURS[0]] + parts[g][NEIGHBOURS[1]])
        for g, (start, width) in enumerate(zip(group_starts, groups)):
            sends[g, DIAGONAL].wait_recv()
            total = (parts[g][0] + parts[g][DIAGONAL]) + from_neighbours[g]
            out_ref[:, pl.ds(start, width)] = total * scale

    dma_sems = pltpu.SemaphoreType.DMA
    return pl.pallas_call(
        kernel_body,
        out_shape=jax.ShapeDtypeStruct((1, n), x.dtype),
        in_specs=[pl.BlockSpec(memory_space=pl.ANY)],
        out_specs=pl.BlockSpec(memory_space=pltpu.VMEM),
        scratch_shapes=[
            [pltpu.VMEM((rows, n), x.dtype) for rows in chunks],
            [pltpu.VMEM((TAIL_ROWS, width), x.dtype) for width in groups],
            pltpu.VMEM((len(NEIGHBOURS), SHARED_ROWS, n), x.dtype),
            [pltpu.VMEM((N_DEV, 1, width), x.dtype) for width in groups],
            dma_sems((len(chunks) + len(groups),)),
            dma_sems((len(NEIGHBOURS),)),
            dma_sems((len(NEIGHBOURS),)),
            dma_sems((len(groups) * len(distances),)),
            dma_sems((len(groups) * len(distances),)),
        ],
        compiler_params=pltpu.CompilerParams(
            collective_id=0,
            disable_semaphore_checks=True,
        ),
    )(x)
```
